```python
import numpy as np

kernel_name = "dist_ag_xy_y_m1024_n512"

def setup_inputs():
    return {"x": np.random.randn(2048, 512).astype(np.float32)}

def reference(x: np.ndarray) -> np.ndarray:
    return x
```

```python
import jax
import jax.numpy as jnp
from jax import lax
from jax.experimental import pallas as pl
from jax.experimental.pallas import tpu as pltpu

MESH = pl.DeviceIdType.MESH

CH = 16
NF = 30
NE = 4
AHEAD = 6
LAG = 4
LOADS = (2, 4, 8, 16, 4)


def pallas_dist_ag_xy_y_m1024_n512_kernel(x: jax.Array):
    m, n = x.shape
    F, E, ny = NF * CH, NE * CH, NF + NE
    assert 2 * F + E == m and sum(LOADS) == ny
    first = [sum(LOADS[:i]) for i in range(len(LOADS))]

    def body(x_hbm, o, sb, ry, rx, ld, ys, yr, xs, xr, lsem):
        mx = lax.axis_index("x")
        my = lax.axis_index("y")
        ynbr = (mx, 1 - my)
        xnbr = (1 - mx, my)
        bar = pltpu.get_barrier_semaphore()
        for nb in (ynbr, xnbr):
            pl.semaphore_signal(bar, inc=1, device_id=nb, device_id_type=MESH)

        fmine = mx * (F + E)
        fother = (1 - mx) * (F + E)
        lbase = my * m
        rbase = (1 - my) * m

        def rows(start, size):
            return pl.ds(start if isinstance(start, int) else pl.multiple_of(start, CH), size)

        def yrow(c):
            return fmine + c * CH if c < NF else c * CH

        def load(g):
            r, sz = yrow(first[g]), LOADS[g] * CH
            return pltpu.make_async_copy(x_hbm.at[rows(r, sz)], o.at[rows(lbase + r, sz)], ld.at[g])

        def ysend(c):
            sl = rows(c * CH, CH)
            return pltpu.make_async_remote_copy(
                sb.at[sl], ry.at[sl], ys, yr.at[c], device_id=ynbr, device_id_type=MESH)

        def xsend(c):
            sl = rows(c * CH, CH)
            return pltpu.make_async_remote_copy(
                ry.at[sl], rx.at[sl], xs, xr.at[c], device_id=xnbr, device_id_type=MESH)

        rest = pltpu.make_async_copy(x_hbm.at[rows(fother, F)], o.at[rows(lbase + fother, F)], lsem)

        for g in range(len(LOADS)):
            load(g).start()

        for i in range(ny + AHEAD + LAG):
            if i < ny:
                if i in first:
                    load(first.index(i)).wait()
                sb[rows(i * CH, CH), :] = o[rows(lbase + yrow(i), CH), :].astype(jnp.bfloat16)
                if i == 0:
                    pl.semaphore_wait(bar, 2)
                ysend(i).start()
                if i == 0:
                    rest.start()
            j = i - AHEAD
            if 0 <= j < ny:
                ysend(j).wait_recv()
                if j < NF:
                    xsend(j).start()
                o[rows(rbase + yrow(j), CH), :] = ry[rows(j * CH, CH), :].astype(jnp.float32)
            k = j - LAG
            if 0 <= k < NF:
                xsend(k).wait_recv()
                o[rows(rbase + fother + k * CH, CH), :] = rx[rows(k * CH, CH), :].astype(jnp.float32)

        pltpu.make_async_copy(sb, sb, ys).wait()
        pltpu.make_async_copy(rx, rx, xs).wait()
        rest.wait()

    return pl.pallas_call(
        body,
        out_shape=jax.ShapeDtypeStruct((2 * m, n), x.dtype),
        in_specs=[pl.BlockSpec(memory_space=pl.ANY)],
        out_specs=pl.BlockSpec(memory_space=pltpu.VMEM),
        scratch_shapes=[
            pltpu.VMEM((F + E, n), jnp.bfloat16),
            pltpu.VMEM((F + E, n), jnp.bfloat16),
            pltpu.VMEM((F, n), jnp.bfloat16),
            pltpu.SemaphoreType.DMA((len(LOADS),)),
            pltpu.SemaphoreType.DMA,
            pltpu.SemaphoreType.DMA((ny,)),
            pltpu.SemaphoreType.DMA,
            pltpu.SemaphoreType.DMA((NF,)),
            pltpu.SemaphoreType.DMA,
        ],
        compiler_params=pltpu.CompilerParams(collective_id=0, disable_semaphore_checks=True),
    )(x)
```

```python
import jax
import jax.numpy as jnp
from jax import lax
from jax.experimental import pallas as pl
from jax.experimental.pallas import tpu as pltpu

MESH = pl.DeviceIdType.MESH

F_CHUNKS = (16,) * 29
E_CHUNKS = (32,) * 3
LOADS = (2, 4, 8, 15, 3)
AHEAD = 6
LAG = 4


def pallas_dist_ag_xy_y_m1024_n512_kernel(x: jax.Array):
    m, n = x.shape
    sizes = F_CHUNKS + E_CHUNKS
    nf, ny = len(F_CHUNKS), len(sizes)
    F, E = sum(F_CHUNKS), sum(E_CHUNKS)
    assert 2 * F + E == m and sum(LOADS) == ny
    offs = [sum(sizes[:i]) for i in range(ny)]
    first = [sum(LOADS[:i]) for i in range(len(LOADS))]

    def body(x_hbm, o, sb, ry, rx, ld, ys, yr, xs, xr, rest_sem, x_ready):
        mx = lax.axis_index("x")
        my = lax.axis_index("y")
        ynbr = (mx, 1 - my)
        xnbr = (1 - mx, my)

        bar = pltpu.get_barrier_semaphore()
        pl.semaphore_signal(bar, inc=1, device_id=ynbr, device_id_type=MESH)

        @pl.when(mx == 0)
        def _():
            pl.semaphore_signal(bar, inc=1, device_id=xnbr, device_id_type=MESH)

        f_mine = mx * (F + E)
        f_other = (1 - mx) * (F + E)
        lbase = my * m
        rbase = (1 - my) * m

        def rows(start, size):
            if not isinstance(start, int):
                start = pl.multiple_of(start, 16)
            return pl.ds(start, size)

        def yrow(c):
            return f_mine + offs[c] if c < nf else offs[c]

        def load(g):
            c = first[g]
            size = sum(sizes[c : c + LOADS[g]])
            return pltpu.make_async_copy(
                x_hbm.at[rows(yrow(c), size)],
                o.at[rows(lbase + yrow(c), size)],
                ld.at[g],
            )

        def ysend(c):
            sl = rows(offs[c], sizes[c])
            return pltpu.make_async_remote_copy(
                sb.at[sl], ry.at[sl], ys, yr.at[c],
                device_id=ynbr, device_id_type=MESH,
            )

        def xsend(c):
            sl = rows(offs[c], sizes[c])
            return pltpu.make_async_remote_copy(
                ry.at[sl], rx.at[sl], xs, xr.at[c],
                device_id=xnbr, device_id_type=MESH,
            )

        rest = pltpu.make_async_copy(
            x_hbm.at[rows(f_other, F)], o.at[rows(lbase + f_other, F)], rest_sem
        )

        def send(c):
            if c in first:
                load(first.index(c)).wait()
            local = o[rows(lbase + yrow(c), sizes[c]), :]
            sb[rows(offs[c], sizes[c]), :] = local.astype(jnp.bfloat16)
            if c == 0:

                @pl.when(mx == 0)
                def _():
                    pl.semaphore_wait(bar, 1)

                @pl.when(mx == 1)
                def _():
                    pl.semaphore_wait(bar, 2)

            ysend(c).start()
            if c == 0:

                @pl.when(mx == 1)
                def _():
                    pl.semaphore_signal(
                        x_ready, inc=1, device_id=xnbr, device_id_type=MESH
                    )

                for g in range(1, len(LOADS)):
                    load(g).start()
                rest.start()

        def recv_y(c):
            ysend(c).wait_recv()
            if c == 0:

                @pl.when(mx == 0)
                def _():
                    pl.semaphore_wait(x_ready, 1)

            if c < nf:
                xsend(c).start()
            got = ry[rows(offs[c], sizes[c]), :]
            o[rows(rbase + yrow(c), sizes[c]), :] = got.astype(o.dtype)

        def recv_x(c):
            xsend(c).wait_recv()
            got = rx[rows(offs[c], sizes[c]), :]
            o[rows(rbase + f_other + offs[c], sizes[c]), :] = got.astype(o.dtype)

        load(0).start()
        for i in range(ny + AHEAD + LAG):
            if i < ny:
                send(i)
            if 0 <= i - AHEAD < ny:
                recv_y(i - AHEAD)
            if 0 <= i - AHEAD - LAG < nf:
                recv_x(i - AHEAD - LAG)

        pltpu.make_async_copy(sb, sb, ys).wait()
        pltpu.make_async_copy(rx, rx, xs).wait()
        rest.wait()

    return pl.pallas_call(
        body,
        out_shape=jax.ShapeDtypeStruct((2 * m, n), x.dtype),
        in_specs=[pl.BlockSpec(memory_space=pl.ANY)],
        out_specs=pl.BlockSpec(memory_space=pltpu.VMEM),
        scratch_shapes=[
            pltpu.VMEM((F + E, n), jnp.bfloat16),
            pltpu.VMEM((F + E, n), jnp.bfloat16),
            pltpu.VMEM((F, n), jnp.bfloat16),
            pltpu.SemaphoreType.DMA((len(LOADS),)),
            pltpu.SemaphoreType.DMA,
            pltpu.SemaphoreType.DMA((ny,)),
            pltpu.SemaphoreType.DMA,
            pltpu.SemaphoreType.DMA((nf,)),
            pltpu.SemaphoreType.DMA,
            pltpu.SemaphoreType.REGULAR,
        ],
        compiler_params=pltpu.CompilerParams(
            collective_id=0, disable_semaphore_checks=True
        ),
    )(x)
```
